```python
import numpy as np

kernel_name = "dist_moe_shared_ep_outshard_n512_d256_e2_h512"

def setup_inputs():
    x = np.random.randn(512, 256).astype(np.float32)
    router_W = np.random.randn(256, 8).astype(np.float32) * 0.1
    scores64 = x.astype(np.float64) @ router_W.astype(np.float64)
    route_idx = np.argsort(-scores64, axis=-1)[:, :1].astype(np.int32)
    expert_W = np.random.randn(8, 256, 512).astype(np.float32) * 0.02
    shared_W = np.random.randn(256, 512).astype(np.float32) * 0.02
    return {"x": x, "router_W": router_W, "route_idx": route_idx, "expert_W": expert_W, "shared_W": shared_W}

def reference(x, router_W, route_idx, expert_W, shared_W):
    scores = x @ router_W
    s_max = scores.max(axis=-1, keepdims=True)
    probs = np.exp(scores - s_max)
    probs = probs / probs.sum(axis=-1, keepdims=True)
    shared = x @ shared_W
    out = np.zeros((512, 512), dtype=np.float32)
    for i in range(512):
        e = int(route_idx[i, 0])
        out[i] = shared[i] + probs[i, e] * (x[i] @ expert_W[e])
    return out
```

```python
import jax
import jax.numpy as jnp
from jax import lax
from jax.experimental import pallas as pl
from jax.experimental.pallas import tpu as pltpu

N_DEV = 4
N_TOK = 512
D_MODEL = 256
H_OUT = 512
N_EXP = 8
E_LOC = N_EXP // N_DEV
BLK = N_TOK // N_DEV


def pallas_dist_moe_shared_ep_outshard_n512_d256_e2_h512_kernel(
    x: jax.Array,
    router_W: jax.Array,
    route_idx: jax.Array,
    expert_W: jax.Array,
    shared_W: jax.Array,
):
    bf16 = jnp.bfloat16
    f32 = jnp.float32

    def body(x_ref, rw_ref, idx_ref, ew_ref, sw_ref, out_ref,
             send_buf, recv_buf, send_sems, recv_sems):
        me = lax.axis_index("i")
        e0 = me * E_LOC
        e1 = e0 + 1
        w0 = ew_ref[0].astype(bf16)
        w1 = ew_ref[1].astype(bf16)

        def expert_part(blk):
            start = pl.multiple_of(blk * BLK, BLK)
            xb = x_ref[pl.ds(start, BLK), :]
            ib = idx_ref[pl.ds(start, BLK), :]
            x0 = jnp.where(ib == e0, xb, 0.0).astype(bf16)
            x1 = jnp.where(ib == e1, xb, 0.0).astype(bf16)
            y = jnp.dot(x0, w0, preferred_element_type=f32)
            y = y + jnp.dot(x1, w1, preferred_element_type=f32)
            return xb, ib, y

        copies = []
        for k in range(1, N_DEV):
            dst = (me + k) % N_DEV
            _, _, y = expert_part(dst)
            send_buf[k - 1] = y.astype(bf16)
            rdma = pltpu.make_async_remote_copy(
                src_ref=send_buf.at[k - 1],
                dst_ref=recv_buf.at[k - 1],
                send_sem=send_sems.at[k - 1],
                recv_sem=recv_sems.at[k - 1],
                device_id=(dst,),
                device_id_type=pl.DeviceIdType.MESH,
            )
            rdma.start()
            copies.append(rdma)

        xb, ib, y_own = expert_part(me)
        scores = jnp.dot(xb, rw_ref[...], preferred_element_type=f32,
                         precision=lax.Precision.HIGHEST)
        s_max = jnp.max(scores, axis=-1, keepdims=True)
        ex = jnp.exp(scores - s_max)
        probs = ex / jnp.sum(ex, axis=-1, keepdims=True)
        lane = lax.broadcasted_iota(jnp.int32, (BLK, N_EXP), 1)
        p = jnp.sum(jnp.where(lane == ib, probs, 0.0), axis=-1, keepdims=True)
        shared = jnp.dot(xb.astype(bf16), sw_ref[...].astype(bf16),
                         preferred_element_type=f32)

        for rdma in copies:
            rdma.wait_send()
        acc = y_own
        for k, rdma in enumerate(copies):
            rdma.wait_recv()
            acc = acc + recv_buf[k].astype(f32)
        out_ref[...] = shared + p * acc

    return pl.pallas_call(
        body,
        out_shape=jax.ShapeDtypeStruct((BLK, H_OUT), jnp.float32),
        scratch_shapes=[
            pltpu.VMEM((N_DEV - 1, BLK, H_OUT), jnp.bfloat16),
            pltpu.VMEM((N_DEV - 1, BLK, H_OUT), jnp.bfloat16),
            pltpu.SemaphoreType.DMA((N_DEV - 1,)),
            pltpu.SemaphoreType.DMA((N_DEV - 1,)),
        ],
    )(x, router_W, route_idx, expert_W, shared_W)
```

```python
import contextlib
import jax
import jax.numpy as jnp
from jax import lax
from jax.experimental import pallas as pl
from jax.experimental.pallas import tpu as pltpu

N_DEV = 4
N_TOK = 512
D_MODEL = 256
H_OUT = 512
N_EXP = 8
E_LOC = N_EXP // N_DEV
BLK = N_TOK // N_DEV
CH = 16
N_CH = BLK // CH
N_GRP = N_DEV - 1
K_ORDER = (2, 1, 3)
SCOPES = False


def _scope(name):
    return jax.named_scope(name) if SCOPES else contextlib.nullcontext()


def _kernel_body(x_hbm, rwt_hbm, idx_hbm, ew_hbm, sw_hbm, out_ref,
                 x_v, rwt_v, idx_v, ew_v, sw_v, xcat_v, acc_v, st_v,
                 send_buf, recv_buf, in_sems, send_sems, recv_sems):
    bf16 = jnp.bfloat16
    f32 = jnp.float32
    i32 = jnp.int32
    me = lax.axis_index("i")
    e0 = me * E_LOC
    e1 = e0 + 1

    cp_idx = pltpu.make_async_copy(idx_hbm, idx_v, in_sems.at[0])
    cp_idx.start()
    cp_xb = []
    for i, k in enumerate(K_ORDER + (0,)):
        c = (me + k) % N_DEV
        rows = pl.ds(pl.multiple_of(c * BLK, BLK), BLK)
        cp_xb.append(pltpu.make_async_copy(x_hbm.at[rows, :], x_v.at[rows, :], in_sems.at[1 + i]))
    for cp in cp_xb[:3]:
        cp.start()
    cp_w0 = pltpu.make_async_copy(ew_hbm.at[pl.ds(0, D_MODEL), :], ew_v.at[pl.ds(0, D_MODEL), :], in_sems.at[5])
    cp_w1 = pltpu.make_async_copy(ew_hbm.at[pl.ds(D_MODEL, D_MODEL), :], ew_v.at[pl.ds(D_MODEL, D_MODEL), :], in_sems.at[6])
    cp_w0.start()
    cp_w1.start()
    cp_xb[3].start()
    cp_rwt = pltpu.make_async_copy(rwt_hbm, rwt_v, in_sems.at[7])
    cp_rwt.start()
    cp_sw = pltpu.make_async_copy(sw_hbm, sw_v, in_sems.at[8])
    cp_sw.start()

    recv_buf[...] = jnp.zeros(recv_buf.shape, recv_buf.dtype)
    barrier = pltpu.get_barrier_semaphore()
    for k in range(1, N_DEV):
        pl.semaphore_signal(barrier, inc=1, device_id=((me + k) % N_DEV,),
                            device_id_type=pl.DeviceIdType.MESH)

    r_i = lax.broadcasted_iota(i32, (BLK, BLK), 0)
    c_i = lax.broadcasted_iota(i32, (BLK, BLK), 1)
    upper = (r_i < c_i).astype(f32).astype(bf16)
    lower = (c_i < r_i).astype(f32).astype(bf16)
    slot_f = r_i.astype(f32)

    with _scope("idxwait"):
        cp_idx.wait()
    rows_k, pos_k, cnt_k, off_k = [], [], [], []
    off = jnp.int32(0)
    with _scope("idxprep"):
        for k in K_ORDER:
            c = (me + k) % N_DEV
            row = idx_v[pl.ds(c, 1), :]
            m = (row >> 1) == me
            cnt = jnp.sum(m.astype(i32))
            m8 = jnp.broadcast_to(m, (8, BLK)).astype(f32).astype(bf16)
            pos = jnp.dot(m8, upper, preferred_element_type=f32)[0:1, :]
            rows_k.append(row)
            pos_k.append(pos)
            cnt_k.append(cnt)
            off_k.append(off)
            off = off + ((cnt + (CH - 1)) // CH) * CH
    total = off

    with _scope("xwait"):
        for cp in cp_xb[:3]:
            cp.wait()
    for g in range(N_GRP):
        @pl.when(g * BLK < total)
        def _(g=g):
            with _scope(f"gather{g}"):
                a0 = jnp.zeros((BLK, D_MODEL), f32)
                a1 = jnp.zeros((BLK, D_MODEL), f32)
                for i, k in enumerate(K_ORDER):
                    c = (me + k) % N_DEV
                    rel = pos_k[i] + (off_k[i] - g * BLK).astype(f32)
                    hit = rel == slot_f
                    s0 = jnp.where(hit & (rows_k[i] == e0), 1.0, 0.0).astype(bf16)
                    s1 = jnp.where(hit & (rows_k[i] == e1), 1.0, 0.0).astype(bf16)
                    xb = x_v[pl.ds(pl.multiple_of(c * BLK, BLK), BLK), :].astype(bf16)
                    a0 = a0 + jnp.dot(s0, xb, preferred_element_type=f32)
                    a1 = a1 + jnp.dot(s1, xb, preferred_element_type=f32)
                xcat_v[g, :, 0:D_MODEL] = a0.astype(bf16)
                xcat_v[g, :, D_MODEL:2 * D_MODEL] = a1.astype(bf16)

    with _scope("w0wait"):
        cp_w0.wait()
    w0 = ew_v[pl.ds(0, D_MODEL), :].astype(bf16)
    for g in range(N_GRP):
        @pl.when(g * BLK < total)
        def _(g=g):
            with _scope(f"mm0_{g}"):
                acc_v[g] = jnp.dot(xcat_v[g, :, 0:D_MODEL], w0, preferred_element_type=f32)
    with _scope("w1wait"):
        cp_w1.wait()
    w1 = ew_v[pl.ds(D_MODEL, D_MODEL), :].astype(bf16)
    for g in range(N_GRP):
        @pl.when(g * BLK < total)
        def _(g=g):
            with _scope(f"mm1_{g}"):
                y = acc_v[g] + jnp.dot(xcat_v[g, :, D_MODEL:2 * D_MODEL], w1,
                                       preferred_element_type=f32)
                send_buf[pl.ds(g * BLK, BLK), :] = y.astype(bf16)

    with _scope("barrier"):
        pl.semaphore_wait(barrier, N_DEV - 1)

    def chunk_copy(i, k, ch):
        src = send_buf.at[pl.ds(pl.multiple_of(off_k[i] + ch * CH, CH), CH), :]
        dst = recv_buf.at[k - 1, pl.ds(pl.multiple_of(ch * CH, CH), CH), :]
        sem = (k - 1) * N_CH + ch
        return pltpu.make_async_remote_copy(
            src_ref=src, dst_ref=dst,
            send_sem=send_sems.at[sem], recv_sem=recv_sems.at[sem],
            device_id=((me + k) % N_DEV,), device_id_type=pl.DeviceIdType.MESH)

    with _scope("sends"):
        for i, k in enumerate(K_ORDER):
            n_ch = (cnt_k[i] + (CH - 1)) // CH

            def start_chunk(ch, carry, i=i, k=k):
                chunk_copy(i, k, ch).start()
                return carry
            lax.fori_loop(0, n_ch, start_chunk, 0)

    with _scope("own"):
        own_row = idx_v[pl.ds(me, 1), :]
        colb = jnp.broadcast_to(own_row, (BLK, BLK)).T
        cp_xb[3].wait()
        xo = x_v[pl.ds(pl.multiple_of(me * BLK, BLK), BLK), :]
        m0 = colb == e0
        m1 = colb == e1
        x0 = jnp.concatenate([jnp.where(m0, xo[:, 0:BLK], 0.0), jnp.where(m0, xo[:, BLK:2 * BLK], 0.0)], axis=1)
        x1 = jnp.concatenate([jnp.where(m1, xo[:, 0:BLK], 0.0), jnp.where(m1, xo[:, BLK:2 * BLK], 0.0)], axis=1)
        acc = jnp.dot(x0.astype(bf16), w0, preferred_element_type=f32)
        acc = acc + jnp.dot(x1.astype(bf16), w1, preferred_element_type=f32)

        cp_rwt.wait()
        scores = lax.dot_general(xo, rwt_v[...], (((1,), (1,)), ((), ())),
                                 precision=lax.Precision.HIGHEST,
                                 preferred_element_type=f32)
        s_max = jnp.max(scores, axis=-1, keepdims=True)
        ex = jnp.exp(scores - s_max)
        probs = ex / jnp.sum(ex, axis=-1, keepdims=True)
        lane8 = lax.broadcasted_iota(i32, (BLK, N_EXP), 1)
        p = jnp.sum(jnp.where(colb[:, 0:N_EXP] == lane8, probs, 0.0), axis=-1, keepdims=True)

        cnt_r = []
        for k in range(1, N_DEV):
            src_dev = (me - k + N_DEV) % N_DEV
            mc = (colb >> 1) == src_dev
            posc = jnp.dot(lower, jnp.where(mc, 1.0, 0.0).astype(bf16), preferred_element_type=f32)
            st_v[k - 1] = jnp.where(mc & (posc == c_i.astype(f32)), 1.0, 0.0).astype(bf16)
            cnt_r.append(jnp.sum(((own_row >> 1) == src_dev).astype(i32)))

        cp_sw.wait()
        shared = jnp.dot(xo.astype(bf16), sw_v[...].astype(bf16), preferred_element_type=f32)

    for k in (1, 3, 2):
        n_r = (cnt_r[k - 1] + (CH - 1)) // CH

        def wait_chunk(ch, carry, k=k):
            chunk_copy(0, k, ch).wait_recv()
            return carry
        with _scope(f"recvwait{k}"):
            lax.fori_loop(0, n_r, wait_chunk, 0)
        with _scope(f"expand{k}"):
            acc = acc + jnp.dot(st_v[k - 1], recv_buf[k - 1], preferred_element_type=f32)

    with _scope("final"):
        out_ref[...] = shared + p * acc

    with _scope("sendwait"):
        for i, k in enumerate(K_ORDER):
            n_ch = (cnt_k[i] + (CH - 1)) // CH

            def wait_send_chunk(ch, carry, i=i, k=k):
                chunk_copy(i, k, ch).wait_send()
                return carry
            lax.fori_loop(0, n_ch, wait_send_chunk, 0)


def pallas_dist_moe_shared_ep_outshard_n512_d256_e2_h512_kernel(
    x: jax.Array,
    router_W: jax.Array,
    route_idx: jax.Array,
    expert_W: jax.Array,
    shared_W: jax.Array,
):
    bf16 = jnp.bfloat16
    f32 = jnp.float32
    idx2 = route_idx.astype(jnp.int32).reshape(N_DEV, BLK)
    rwt = router_W.T
    ew2 = expert_W.reshape(E_LOC * D_MODEL, H_OUT)
    any_spec = pl.BlockSpec(memory_space=pl.ANY)
    return pl.pallas_call(
        _kernel_body,
        out_shape=jax.ShapeDtypeStruct((BLK, H_OUT), f32),
        in_specs=[any_spec] * 5,
        scratch_shapes=[
            pltpu.VMEM((N_TOK, D_MODEL), f32),
            pltpu.VMEM((N_EXP, D_MODEL), f32),
            pltpu.VMEM((N_DEV, BLK), jnp.int32),
            pltpu.VMEM((E_LOC * D_MODEL, H_OUT), f32),
            pltpu.VMEM((D_MODEL, H_OUT), f32),
            pltpu.VMEM((N_GRP, BLK, E_LOC * D_MODEL), bf16),
            pltpu.VMEM((N_GRP, BLK, H_OUT), f32),
            pltpu.VMEM((N_DEV - 1, BLK, BLK), bf16),
            pltpu.VMEM((N_GRP * BLK, H_OUT), bf16),
            pltpu.VMEM((N_DEV - 1, BLK, H_OUT), bf16),
            pltpu.SemaphoreType.DMA((9,)),
            pltpu.SemaphoreType.DMA(((N_DEV - 1) * N_CH,)),
            pltpu.SemaphoreType.DMA(((N_DEV - 1) * N_CH,)),
        ],
        compiler_params=pltpu.CompilerParams(collective_id=0),
    )(x, rwt, idx2, ew2, shared_W)
```

```python
import contextlib
import jax
import jax.numpy as jnp
from jax import lax
from jax.experimental import pallas as pl
from jax.experimental.pallas import tpu as pltpu

N_DEV = 4
N_TOK = 512
D_MODEL = 256
H_OUT = 512
N_EXP = 8
E_LOC = N_EXP // N_DEV
BLK = N_TOK // N_DEV
CH = 16
N_CH = BLK // CH
GM = 144
N_GRP = -(-(N_DEV - 1) * BLK // GM)
K_ORDER = (2, 1, 3)
NQ = 4
QW = H_OUT // NQ
SCOPES = False


def _scope(name):
    return jax.named_scope(name) if SCOPES else contextlib.nullcontext()


def _kernel_body(x_hbm, rwt_hbm, idx_hbm, ew_hbm, sw_hbm, out_ref,
                 x_v, rwt_v, idx_v, ew_v, sw_v, xcat_v, wb_v, st_v,
                 send_buf, recv_buf, in_sems, send_sems, recv_sems):
    bf16 = jnp.bfloat16
    f32 = jnp.float32
    i32 = jnp.int32
    me = lax.axis_index("i")
    e0 = me * E_LOC
    e1 = e0 + 1

    cp_idx = pltpu.make_async_copy(idx_hbm, idx_v, in_sems.at[0])
    cp_idx.start()
    cp_xb = []
    for i, k in enumerate(K_ORDER + (0,)):
        c = (me + k) % N_DEV
        rows = pl.ds(pl.multiple_of(c * BLK, BLK), BLK)
        cp_xb.append(pltpu.make_async_copy(x_hbm.at[rows, :], x_v.at[rows, :], in_sems.at[1 + i]))
    for cp in cp_xb[:3]:
        cp.start()
    cp_wq = []
    for q in range(NQ):
        cols = pl.ds(q * QW, QW)
        cp_wq.append(pltpu.make_async_copy(ew_hbm.at[:, cols], ew_v.at[:, cols], in_sems.at[8 + q]))
        cp_wq[-1].start()
    cp_xb[3].start()
    cp_rwt = pltpu.make_async_copy(rwt_hbm, rwt_v, in_sems.at[5])
    cp_rwt.start()
    cp_sw = pltpu.make_async_copy(sw_hbm, sw_v, in_sems.at[6])
    cp_sw.start()

    recv_buf[...] = jnp.zeros(recv_buf.shape, recv_buf.dtype)
    barrier = pltpu.get_barrier_semaphore()
    for k in range(1, N_DEV):
        pl.semaphore_signal(barrier, inc=1, device_id=((me + k) % N_DEV,),
                            device_id_type=pl.DeviceIdType.MESH)

    r_i = lax.broadcasted_iota(i32, (BLK, BLK), 0)
    c_i = lax.broadcasted_iota(i32, (BLK, BLK), 1)
    upper = (r_i < c_i).astype(f32).astype(bf16)
    lower = (c_i < r_i).astype(f32).astype(bf16)
    slot_f = lax.broadcasted_iota(i32, (GM, BLK), 0).astype(f32)

    with _scope("idxwait"):
        cp_idx.wait()
    rows_k, pos_k, cnt_k, off_k = [], [], [], []
    off = jnp.int32(0)
    with _scope("idxprep"):
        for k in K_ORDER:
            c = (me + k) % N_DEV
            row = idx_v[pl.ds(c, 1), :]
            m = (row >> 1) == me
            cnt = jnp.sum(m.astype(i32))
            m8 = jnp.broadcast_to(m, (8, BLK)).astype(f32).astype(bf16)
            pos = jnp.dot(m8, upper, preferred_element_type=f32)[0:1, :]
            rows_k.append(row)
            pos_k.append(pos)
            cnt_k.append(cnt)
            off_k.append(off)
            off = off + ((cnt + (CH - 1)) // CH) * CH
    total = off

    with _scope("xwait"):
        for cp in cp_xb[:3]:
            cp.wait()
    for g in range(N_GRP):
        @pl.when(g * GM < total)
        def _(g=g):
            with _scope(f"gather{g}"):
                a0 = jnp.zeros((GM, D_MODEL), f32)
                a1 = jnp.zeros((GM, D_MODEL), f32)
                for i, k in enumerate(K_ORDER):
                    c = (me + k) % N_DEV
                    rel = pos_k[i] + (off_k[i] - g * GM).astype(f32)
                    hit = rel == slot_f
                    s0 = jnp.where(hit & (rows_k[i] == e0), 1.0, 0.0).astype(bf16)
                    s1 = jnp.where(hit & (rows_k[i] == e1), 1.0, 0.0).astype(bf16)
                    xb = x_v[pl.ds(pl.multiple_of(c * BLK, BLK), BLK), :].astype(bf16)
                    a0 = a0 + jnp.dot(s0, xb, preferred_element_type=f32)
                    a1 = a1 + jnp.dot(s1, xb, preferred_element_type=f32)
                xcat_v[g, :, 0:D_MODEL] = a0.astype(bf16)
                xcat_v[g, :, D_MODEL:2 * D_MODEL] = a1.astype(bf16)

    def chunk_copy(i, k, ch, q):
        rows_s = pl.ds(pl.multiple_of(off_k[i] + ch * CH, CH), CH)
        rows_d = pl.ds(pl.multiple_of((k - 1) * BLK + ch * CH, CH), CH)
        cols = pl.ds(q * QW, QW)
        sem = ((k - 1) * N_CH + ch) * NQ + q
        return pltpu.make_async_remote_copy(
            src_ref=send_buf.at[rows_s, cols], dst_ref=recv_buf.at[rows_d, cols],
            send_sem=send_sems.at[sem], recv_sem=recv_sems.at[sem],
            device_id=((me + k) % N_DEV,), device_id_type=pl.DeviceIdType.MESH)

    for q in range(NQ):
        with _scope(f"wwait{q}"):
            cp_wq[q].wait()
        with _scope(f"mm{q}"):
            wq = ew_v[:, pl.ds(q * QW, QW)].astype(bf16)
            wb_v[:, pl.ds(q * QW, QW)] = wq
            for g in range(N_GRP):
                @pl.when(g * GM < total)
                def _(g=g, q=q, wq=wq):
                    y = jnp.dot(xcat_v[g], wq, preferred_element_type=f32)
                    send_buf[pl.ds(g * GM, GM), pl.ds(q * QW, QW)] = y.astype(bf16)
        if q == 0:
            with _scope("barrier"):
                pl.semaphore_wait(barrier, N_DEV - 1)
        with _scope(f"sends{q}"):
            for i, k in enumerate(K_ORDER):
                n_ch = (cnt_k[i] + (CH - 1)) // CH

                def start_chunk(ch, carry, i=i, k=k, q=q):
                    chunk_copy(i, k, ch, q).start()
                    return carry
                lax.fori_loop(0, n_ch, start_chunk, 0)

    with _scope("own"):
        own_row = idx_v[pl.ds(me, 1), :]
        colb = jnp.broadcast_to(own_row, (BLK, BLK)).T
        cp_xb[3].wait()
        xo = x_v[pl.ds(pl.multiple_of(me * BLK, BLK), BLK), :]
        m0 = colb == e0
        m1 = colb == e1
        x0 = jnp.concatenate([jnp.where(m0, xo[:, 0:BLK], 0.0), jnp.where(m0, xo[:, BLK:2 * BLK], 0.0)], axis=1)
        x1 = jnp.concatenate([jnp.where(m1, xo[:, 0:BLK], 0.0), jnp.where(m1, xo[:, BLK:2 * BLK], 0.0)], axis=1)
        acc = jnp.dot(x0.astype(bf16), wb_v[pl.ds(0, D_MODEL), :], preferred_element_type=f32)
        acc = acc + jnp.dot(x1.astype(bf16), wb_v[pl.ds(D_MODEL, D_MODEL), :], preferred_element_type=f32)

        cp_rwt.wait()
        scores = lax.dot_general(xo, rwt_v[...], (((1,), (1,)), ((), ())),
                                 precision=lax.Precision.HIGHEST,
                                 preferred_element_type=f32)
        s_max = jnp.max(scores, axis=-1, keepdims=True)
        ex = jnp.exp(scores - s_max)
        probs = ex / jnp.sum(ex, axis=-1, keepdims=True)
        lane8 = lax.broadcasted_iota(i32, (BLK, N_EXP), 1)
        p = jnp.sum(jnp.where(colb[:, 0:N_EXP] == lane8, probs, 0.0), axis=-1, keepdims=True)

        cnt_r = []
        for k in range(1, N_DEV):
            src_dev = (me - k + N_DEV) % N_DEV
            mc = (colb >> 1) == src_dev
            posc = jnp.dot(lower, jnp.where(mc, 1.0, 0.0).astype(bf16), preferred_element_type=f32)
            st_v[:, pl.ds((k - 1) * BLK, BLK)] = jnp.where(mc & (posc == c_i.astype(f32)), 1.0, 0.0).astype(bf16)
            cnt_r.append(jnp.sum(((own_row >> 1) == src_dev).astype(i32)))

        cp_sw.wait()
        shared = jnp.dot(xo.astype(bf16), sw_v[...].astype(bf16), preferred_element_type=f32)
        out_ref[...] = shared + p * acc

    for q in range(NQ):
        for k in (1, 3, 2):
            n_r = (cnt_r[k - 1] + (CH - 1)) // CH

            def wait_chunk(ch, carry, k=k, q=q):
                chunk_copy(0, k, ch, q).wait_recv()
                return carry
            with _scope(f"recvwait{k}_{q}"):
                lax.fori_loop(0, n_r, wait_chunk, 0)
        with _scope(f"expand_{q}"):
            cols = pl.ds(q * QW, QW)
            contrib = jnp.dot(st_v[...], recv_buf[:, cols], preferred_element_type=f32)
            out_ref[:, cols] = out_ref[:, cols] + p * contrib

    with _scope("sendwait"):
        for i, k in enumerate(K_ORDER):
            n_ch = (cnt_k[i] + (CH - 1)) // CH

            def wait_send_chunk(ch, carry, i=i, k=k):
                for q in range(NQ):
                    chunk_copy(i, k, ch, q).wait_send()
                return carry
            lax.fori_loop(0, n_ch, wait_send_chunk, 0)


def pallas_dist_moe_shared_ep_outshard_n512_d256_e2_h512_kernel(
    x: jax.Array,
    router_W: jax.Array,
    route_idx: jax.Array,
    expert_W: jax.Array,
    shared_W: jax.Array,
):
    bf16 = jnp.bfloat16
    f32 = jnp.float32
    idx2 = route_idx.astype(jnp.int32).reshape(N_DEV, BLK)
    rwt = router_W.T
    ew2 = expert_W.reshape(E_LOC * D_MODEL, H_OUT)
    any_spec = pl.BlockSpec(memory_space=pl.ANY)
    return pl.pallas_call(
        _kernel_body,
        out_shape=jax.ShapeDtypeStruct((BLK, H_OUT), f32),
        in_specs=[any_spec] * 5,
        scratch_shapes=[
            pltpu.VMEM((N_TOK, D_MODEL), f32),
            pltpu.VMEM((N_EXP, D_MODEL), f32),
            pltpu.VMEM((N_DEV, BLK), jnp.int32),
            pltpu.VMEM((E_LOC * D_MODEL, H_OUT), f32),
            pltpu.VMEM((D_MODEL, H_OUT), f32),
            pltpu.VMEM((N_GRP, GM, E_LOC * D_MODEL), bf16),
            pltpu.VMEM((E_LOC * D_MODEL, H_OUT), bf16),
            pltpu.VMEM((BLK, (N_DEV - 1) * BLK), bf16),
            pltpu.VMEM((N_GRP * GM, H_OUT), bf16),
            pltpu.VMEM(((N_DEV - 1) * BLK, H_OUT), bf16),
            pltpu.SemaphoreType.DMA((8 + NQ,)),
            pltpu.SemaphoreType.DMA(((N_DEV - 1) * N_CH * NQ,)),
            pltpu.SemaphoreType.DMA(((N_DEV - 1) * N_CH * NQ,)),
        ],
        compiler_params=pltpu.CompilerParams(collective_id=0, disable_semaphore_checks=True),
    )(x, rwt, idx2, ew2, shared_W)
```

```python
import jax
import jax.numpy as jnp
from jax import lax
from jax.experimental import pallas as pl
from jax.experimental.pallas import tpu as pltpu

N_DEV = 4
N_TOK = 512
D_MODEL = 256
H_OUT = 512
N_EXP = 8
E_LOC = N_EXP // N_DEV
BLK = N_TOK // N_DEV
CH = 16
N_CH = BLK // CH
GM = 144
N_GRP = -(-(N_DEV - 1) * BLK // GM)
K_ORDER = (2, 1, 3)
NQ = 4
QW = H_OUT // NQ


def _kernel_body(x_hbm, rwt_hbm, idx_hbm, ew_hbm, sw_hbm, out_ref,
                 x_v, rwt_v, idx_v, ew_v, sw_v, xcat_v, st_v,
                 send_buf, recv_buf, in_sems, send_sems, recv_sems):
    bf16 = jnp.bfloat16
    f32 = jnp.float32
    i32 = jnp.int32
    me = lax.axis_index("i")
    e0 = me * E_LOC
    e1 = e0 + 1

    cp_idx = pltpu.make_async_copy(idx_hbm, idx_v, in_sems.at[0])
    cp_idx.start()
    cp_xb = []
    for i, k in enumerate(K_ORDER + (0,)):
        c = (me + k) % N_DEV
        rows = pl.ds(pl.multiple_of(c * BLK, BLK), BLK)
        cp_xb.append(pltpu.make_async_copy(x_hbm.at[rows, :], x_v.at[rows, :], in_sems.at[1 + i]))
    for cp in cp_xb[:3]:
        cp.start()
    cp_wq = []
    for q in range(NQ):
        cols = pl.ds(q * QW, QW)
        cp_wq.append(pltpu.make_async_copy(ew_hbm.at[:, cols], ew_v.at[:, cols], in_sems.at[7 + q]))
        cp_wq[-1].start()
    cp_xb[3].start()
    cp_rwt = pltpu.make_async_copy(rwt_hbm, rwt_v, in_sems.at[5])
    cp_rwt.start()
    cp_sw = pltpu.make_async_copy(sw_hbm, sw_v, in_sems.at[6])
    cp_sw.start()

    recv_buf[...] = jnp.zeros(recv_buf.shape, recv_buf.dtype)
    barrier = pltpu.get_barrier_semaphore()
    for k in range(1, N_DEV):
        pl.semaphore_signal(barrier, inc=1, device_id=((me + k) % N_DEV,),
                            device_id_type=pl.DeviceIdType.MESH)

    r_i = lax.broadcasted_iota(i32, (BLK, BLK), 0)
    c_i = lax.broadcasted_iota(i32, (BLK, BLK), 1)
    upper = (r_i < c_i).astype(f32).astype(bf16)
    lower = (c_i < r_i).astype(f32).astype(bf16)
    slot_f = lax.broadcasted_iota(i32, (GM, BLK), 0).astype(f32)

    cp_idx.wait()
    rows_k, pos_k, cnt_k, off_k = [], [], [], []
    off = jnp.int32(0)
    for k in K_ORDER:
        c = (me + k) % N_DEV
        row = idx_v[pl.ds(c, 1), :]
        m = (row >> 1) == me
        cnt = jnp.sum(m.astype(i32))
        m8 = jnp.broadcast_to(m, (8, BLK)).astype(f32).astype(bf16)
        pos = jnp.dot(m8, upper, preferred_element_type=f32)[0:1, :]
        rows_k.append(row)
        pos_k.append(pos)
        cnt_k.append(cnt)
        off_k.append(off)
        off = off + ((cnt + (CH - 1)) // CH) * CH
    total = off

    for cp in cp_xb[:3]:
        cp.wait()
    for g in range(N_GRP):
        @pl.when(g * GM < total)
        def _(g=g):
            a0 = jnp.zeros((GM, D_MODEL), f32)
            a1 = jnp.zeros((GM, D_MODEL), f32)
            for i, k in enumerate(K_ORDER):
                c = (me + k) % N_DEV
                rel = pos_k[i] + (off_k[i] - g * GM).astype(f32)
                hit = rel == slot_f
                s0 = jnp.where(hit & (rows_k[i] == e0), 1.0, 0.0).astype(bf16)
                s1 = jnp.where(hit & (rows_k[i] == e1), 1.0, 0.0).astype(bf16)
                xb = x_v[pl.ds(pl.multiple_of(c * BLK, BLK), BLK), :].astype(bf16)
                a0 = a0 + jnp.dot(s0, xb, preferred_element_type=f32)
                a1 = a1 + jnp.dot(s1, xb, preferred_element_type=f32)
            xcat_v[g, :, 0:D_MODEL] = a0.astype(bf16)
            xcat_v[g, :, D_MODEL:2 * D_MODEL] = a1.astype(bf16)

    def chunk_copy(i, k, ch, q):
        rows_s = pl.ds(pl.multiple_of(off_k[i] + ch * CH, CH), CH)
        rows_d = pl.ds(pl.multiple_of((k - 1) * BLK + ch * CH, CH), CH)
        cols = pl.ds(q * QW, QW)
        sem = ((k - 1) * N_CH + ch) * NQ + q
        return pltpu.make_async_remote_copy(
            src_ref=send_buf.at[rows_s, cols], dst_ref=recv_buf.at[rows_d, cols],
            send_sem=send_sems.at[sem], recv_sem=recv_sems.at[sem],
            device_id=((me + k) % N_DEV,), device_id_type=pl.DeviceIdType.MESH)

    def chunk_loop(cnt, fn):
        def body(ch, carry):
            fn(ch)
            return carry
        lax.fori_loop(0, (cnt + (CH - 1)) // CH, body, 0)

    for q in range(NQ):
        cp_wq[q].wait()
        wq = ew_v[:, pl.ds(q * QW, QW)].astype(bf16)
        for g in range(N_GRP):
            @pl.when(g * GM < total)
            def _(g=g, q=q, wq=wq):
                y = jnp.dot(xcat_v[g], wq, preferred_element_type=f32)
                send_buf[pl.ds(g * GM, GM), pl.ds(q * QW, QW)] = y.astype(bf16)
        if q == 0:
            pl.semaphore_wait(barrier, N_DEV - 1)
        for i, k in enumerate(K_ORDER):
            chunk_loop(cnt_k[i], lambda ch, i=i, k=k, q=q: chunk_copy(i, k, ch, q).start())

    own_row = idx_v[pl.ds(me, 1), :]
    colb = jnp.broadcast_to(own_row, (BLK, BLK)).T
    cp_xb[3].wait()
    xo = x_v[pl.ds(pl.multiple_of(me * BLK, BLK), BLK), :]
    m0 = colb == e0
    m1 = colb == e1
    x0 = jnp.concatenate([jnp.where(m0, xo[:, 0:BLK], 0.0),
                          jnp.where(m0, xo[:, BLK:2 * BLK], 0.0)], axis=1)
    x1 = jnp.concatenate([jnp.where(m1, xo[:, 0:BLK], 0.0),
                          jnp.where(m1, xo[:, BLK:2 * BLK], 0.0)], axis=1)
    acc = jnp.dot(x0.astype(bf16), ew_v[pl.ds(0, D_MODEL), :].astype(bf16),
                  preferred_element_type=f32)
    acc = acc + jnp.dot(x1.astype(bf16), ew_v[pl.ds(D_MODEL, D_MODEL), :].astype(bf16),
                        preferred_element_type=f32)

    cp_rwt.wait()
    scores = lax.dot_general(xo, rwt_v[...], (((1,), (1,)), ((), ())),
                             precision=lax.Precision.HIGHEST,
                             preferred_element_type=f32)
    s_max = jnp.max(scores, axis=-1, keepdims=True)
    ex = jnp.exp(scores - s_max)
    probs = ex / jnp.sum(ex, axis=-1, keepdims=True)
    lane8 = lax.broadcasted_iota(i32, (BLK, N_EXP), 1)
    p = jnp.sum(jnp.where(colb[:, 0:N_EXP] == lane8, probs, 0.0), axis=-1, keepdims=True)

    cnt_r = []
    for k in range(1, N_DEV):
        src_dev = (me - k + N_DEV) % N_DEV
        mc = (colb >> 1) == src_dev
        posc = jnp.dot(lower, jnp.where(mc, 1.0, 0.0).astype(bf16), preferred_element_type=f32)
        st_v[:, pl.ds((k - 1) * BLK, BLK)] = jnp.where(
            mc & (posc == c_i.astype(f32)), 1.0, 0.0).astype(bf16)
        cnt_r.append(jnp.sum(((own_row >> 1) == src_dev).astype(i32)))

    cp_sw.wait()
    shared = jnp.dot(xo.astype(bf16), sw_v[...].astype(bf16), preferred_element_type=f32)
    out_ref[...] = shared + p * acc

    for q in range(NQ):
        if q == NQ - 1:
            for i, k in enumerate(K_ORDER):
                for qq in range(NQ):
                    chunk_loop(cnt_k[i], lambda ch, i=i, k=k, qq=qq: chunk_copy(i, k, ch, qq).wait_send())
        for k in (1, 3, 2):
            chunk_loop(cnt_r[k - 1], lambda ch, k=k, q=q: chunk_copy(0, k, ch, q).wait_recv())
        cols = pl.ds(q * QW, QW)
        contrib = jnp.dot(st_v[...], recv_buf[:, cols], preferred_element_type=f32)
        out_ref[:, cols] = out_ref[:, cols] + p * contrib


def pallas_dist_moe_shared_ep_outshard_n512_d256_e2_h512_kernel(
    x: jax.Array,
    router_W: jax.Array,
    route_idx: jax.Array,
    expert_W: jax.Array,
    shared_W: jax.Array,
):
    bf16 = jnp.bfloat16
    f32 = jnp.float32
    idx2 = route_idx.astype(jnp.int32).reshape(N_DEV, BLK)
    rwt = router_W.T
    ew2 = expert_W.reshape(E_LOC * D_MODEL, H_OUT)
    any_spec = pl.BlockSpec(memory_space=pl.ANY)
    return pl.pallas_call(
        _kernel_body,
        out_shape=jax.ShapeDtypeStruct((BLK, H_OUT), f32),
        in_specs=[any_spec] * 5,
        scratch_shapes=[
            pltpu.VMEM((N_TOK, D_MODEL), f32),
            pltpu.VMEM((N_EXP, D_MODEL), f32),
            pltpu.VMEM((N_DEV, BLK), jnp.int32),
            pltpu.VMEM((E_LOC * D_MODEL, H_OUT), f32),
            pltpu.VMEM((D_MODEL, H_OUT), f32),
            pltpu.VMEM((N_GRP, GM, E_LOC * D_MODEL), bf16),
            pltpu.VMEM((BLK, (N_DEV - 1) * BLK), bf16),
            pltpu.VMEM((N_GRP * GM, H_OUT), bf16),
            pltpu.VMEM(((N_DEV - 1) * BLK, H_OUT), bf16),
            pltpu.SemaphoreType.DMA((7 + NQ,)),
            pltpu.SemaphoreType.DMA(((N_DEV - 1) * N_CH * NQ,)),
            pltpu.SemaphoreType.DMA(((N_DEV - 1) * N_CH * NQ,)),
        ],
        compiler_params=pltpu.CompilerParams(collective_id=0, disable_semaphore_checks=True),
    )(x, rwt, idx2, ew2, shared_W)
```
